```python
import numpy as np

kernel_name = "dist_matmul_mk_i_outk_m1024_n1024_k512"

def setup_inputs():
    A = np.random.randn(1024, 2048).astype(np.float32)
    B = np.random.randn(2048, 1024).astype(np.float32)
    return {"A": A, "B": B}

def reference(A: np.ndarray, B: np.ndarray) -> np.ndarray:
    return A @ B
```

```python
import contextlib
import jax
import jax.numpy as jnp
from jax import lax
from jax.experimental import pallas as pl
from jax.experimental.pallas import tpu as pltpu

N_DEV = 4
T = 128
SCOPES = False
NF = 3


def scope(name):
    return jax.named_scope(name) if SCOPES else contextlib.nullcontext()


def pallas_dist_matmul_mk_i_outk_m1024_n1024_k512_kernel(A, B):
    m, k = A.shape
    _, n = B.shape
    mb = m // N_DEV
    hb = mb // 2
    qb = hb // 2
    nt = n // T
    nu = 2 * nt
    nb = nu - NF
    bf16 = jnp.bfloat16
    f32 = jnp.float32

    k0_sends = [(0, 1), (1, 2), (2, 3), (3, 4)] + [(u, min(u + 2, nb)) for u in range(4, nb, 2)]
    k1_sends = [(0, 8), (8, nb), (nb, nu)]
    k2_sends = [(0, 8), (8, 12), (12, 14), (14, 16)]
    sends = [k0_sends, k1_sends, k2_sends]
    sem_base = [0, len(k0_sends), len(k0_sends) + len(k1_sends)]
    n_rdma = sum(len(c) for c in sends)

    def body(a_hbm, b_hbm, o_ref, ad_vm, a_vm, b_vm, b_bf, send_r, send_l, recv_l, recv_r,
             extra_l, extra_r, a_sems, b_sems, sr_sems, sl_sems, rl_sems, rr_sems, fs_sems, fr_sems):
        me = lax.axis_index("i")
        right = (me + 1) & (N_DEV - 1)
        left = (me + N_DEV - 1) & (N_DEV - 1)
        diag = me ^ 2

        def ad_copy(q):
            return pltpu.make_async_copy(a_hbm.at[diag, :, q], ad_vm.at[q], a_sems.at[q])

        a_src = [(right, 1), (left, 0), (right, 0), (left, 1), (me, 0), (me, 1)]

        def a_copy(s):
            blk, h = a_src[s]
            return pltpu.make_async_copy(a_hbm.at[blk, h], a_vm.at[s], a_sems.at[2 + s])

        def b_copy(c):
            return pltpu.make_async_copy(b_hbm.at[:, pl.ds(c * T, T)], b_vm.at[c], b_sems.at[c])

        def remote(src, dst, ssem, rsem, dev):
            return pltpu.make_async_remote_copy(src_ref=src, dst_ref=dst, send_sem=ssem, recv_sem=rsem,
                                                device_id=(dev,), device_id_type=pl.DeviceIdType.MESH)

        def rdma(d, p, j):
            u0, u1 = sends[p][j]
            s = sem_base[p] + j
            idx = (p, pl.ds(u0, u1 - u0))
            if d == "r":
                return remote(send_r.at[idx], recv_l.at[idx], sr_sems.at[s], rl_sems.at[s], right)
            return remote(send_l.at[idx], recv_r.at[idx], sl_sems.at[s], rr_sems.at[s], left)

        fl = (0, pl.ds(nb, NF))
        flex_h0_def = lambda: remote(send_r.at[fl], recv_l.at[fl], fs_sems.at[0], fr_sems.at[0], right)
        flex_h0_alt = lambda: remote(send_r.at[fl], extra_r, fs_sems.at[0], fr_sems.at[3], left)
        flex_h1_def = lambda: remote(send_l.at[fl], recv_r.at[fl], fs_sems.at[1], fr_sems.at[1], left)
        flex_h1_alt = lambda: remote(send_l.at[fl], extra_l, fs_sems.at[1], fr_sems.at[2], right)

        def start(p, j):
            with scope("start_k%d_%d" % (p, j)):
                rdma("r", p, j).start()
                rdma("l", p, j).start()

        def b_cols(c0, c1):
            return jnp.concatenate([b_bf[c] for c in range(c0, c1)], axis=1) if c1 - c0 > 1 else b_bf[c0]

        barrier = pltpu.get_barrier_semaphore()

        b_copy(0).start()
        ad_copy(0).start()
        pl.semaphore_signal(barrier, inc=1, device_id=(left,), device_id_type=pl.DeviceIdType.MESH)
        ad_copy(1).start()
        pl.semaphore_signal(barrier, inc=1, device_id=(right,), device_id_type=pl.DeviceIdType.MESH)
        for c in range(1, nt):
            b_copy(c).start()

        @pl.when(me == 0)
        def _():
            recv_l[0, pl.ds(nb, NF)] = jnp.zeros((NF, qb, T), bf16)
            recv_r[0, pl.ds(nb, NF)] = jnp.zeros((NF, qb, T), bf16)

        @pl.when(me != 2)
        def _():
            extra_l[...] = jnp.zeros((NF, qb, T), bf16)
            extra_r[...] = jnp.zeros((NF, qb, T), bf16)

        def diag_piece(q, c):
            res = jnp.dot(ad_vm[q].reshape(hb, k).astype(bf16), b_bf[c], preferred_element_type=f32).astype(bf16)
            send_r[0, 2 * c + q] = res[:qb]
            send_l[0, 2 * c + q] = res[qb:]

        with scope("wait_b0"):
            b_copy(0).wait()
        for s in range(6):
            a_copy(s).start()
        b_bf[0] = b_vm[0].astype(bf16)
        with scope("wait_ad0"):
            ad_copy(0).wait()
        diag_piece(0, 0)
        with scope("wait_barrier"):
            pl.semaphore_wait(barrier, 2)
        start(0, 0)
        with scope("wait_ad1"):
            ad_copy(1).wait()
        diag_piece(1, 0)
        start(0, 1)
        with scope("wait_b1"):
            b_copy(1).wait()
        b_bf[1] = b_vm[1].astype(bf16)
        diag_piece(0, 1)
        start(0, 2)
        diag_piece(1, 1)
        start(0, 3)
        for c in range(2, nt):
            with scope("wait_b%d" % c):
                b_copy(c).wait()
            b_bf[c] = b_vm[c].astype(bf16)
            res = jnp.dot(ad_vm[...].reshape(mb, k).astype(bf16), b_bf[c], preferred_element_type=f32).astype(bf16)
            send_r[0, 2 * c] = res[0 * qb:1 * qb]
            send_l[0, 2 * c] = res[1 * qb:2 * qb]
            send_r[0, 2 * c + 1] = res[2 * qb:3 * qb]
            send_l[0, 2 * c + 1] = res[3 * qb:4 * qb]
            if c + 2 < len(k0_sends):
                start(0, c + 2)

        with scope("start_flex"):
            @pl.when(me != 3)
            def _():
                flex_h0_def().start()

            @pl.when(me == 3)
            def _():
                flex_h0_alt().start()

            @pl.when(me != 1)
            def _():
                flex_h1_def().start()

            @pl.when(me == 1)
            def _():
                flex_h1_alt().start()

        def units(res, c0, c1):
            for c in range(c0, c1):
                cc = slice((c - c0) * T, (c - c0 + 1) * T)
                for q in range(2):
                    yield 2 * c + q, res[q * qb:(q + 1) * qb, cc], res[hb + q * qb:hb + (q + 1) * qb, cc]

        with scope("wait_a01"):
            a_copy(0).wait()
            a_copy(1).wait()
        cf = nb // 2
        for j, (c0, c1) in enumerate([(0, 4), (4, (nb + 1) // 2)]):
            res = jnp.dot(a_vm[pl.ds(0, 2)].reshape(mb, k).astype(bf16), b_cols(c0, c1),
                          preferred_element_type=f32)
            for u, pr, plft in units(res, c0, c1):
                if u < nb:
                    send_r[1, u] = pr.astype(bf16)
                    send_l[1, u] = plft.astype(bf16)
            start(1, j)

        with scope("wait_a45"):
            a_copy(4).wait()
            a_copy(5).wait()
        o_ref[...] = jnp.dot(a_vm[pl.ds(4, 2)].reshape(mb, k).astype(bf16), b_cols(0, nt), preferred_element_type=f32)

        with scope("wait_a23"):
            a_copy(2).wait()
            a_copy(3).wait()
        with scope("recv_k0"):
            for j in range(len(k0_sends)):
                rdma("r", 0, j).wait_recv()
                rdma("l", 0, j).wait_recv()

            @pl.when(me != 0)
            def _():
                flex_h0_def().wait_recv()
                flex_h1_def().wait_recv()

            @pl.when(me == 2)
            def _():
                flex_h0_alt().wait_recv()
                flex_h1_alt().wait_recv()

        res = jnp.dot(a_vm[pl.ds(0, 2)].reshape(mb, k).astype(bf16), b_cols(cf, nt), preferred_element_type=f32)
        for u, pr, plft in units(res, cf, nt):
            if u >= nb:
                send_r[1, u] = (pr + extra_l[u - nb].astype(f32)).astype(bf16)
                send_l[1, u] = (plft + extra_r[u - nb].astype(f32)).astype(bf16)
        start(1, 2)

        for j, (u0, u1) in enumerate(k2_sends):
            c0, c1 = u0 // 2, u1 // 2
            res = jnp.dot(a_vm[pl.ds(2, 2)].reshape(mb, k).astype(bf16), b_cols(c0, c1), preferred_element_type=f32)
            for u, pr, plft in units(res, c0, c1):
                send_r[2, u] = (pr + recv_l[0, u].astype(f32)).astype(bf16)
                send_l[2, u] = (plft + recv_r[0, u].astype(f32)).astype(bf16)
            start(2, j)

        def accumulate(buf, p, u0, u1, half):
            for u in range(u0, u1):
                rows = pl.ds(half * hb + (u % 2) * qb, qb)
                cols = pl.ds((u // 2) * T, T)
                o_ref[rows, cols] += buf[p, u].astype(f32)

        for j, (u0, u1) in enumerate(k1_sends):
            with scope("recv_k1_%d" % j):
                rdma("r", 1, j).wait_recv()
                rdma("l", 1, j).wait_recv()
            accumulate(recv_r, 1, u0, u1, 0)
            accumulate(recv_l, 1, u0, u1, 1)

        for p in range(2):
            for j in range(len(sends[p])):
                rdma("r", p, j).wait_send()
                rdma("l", p, j).wait_send()
        flex_h0_def().wait_send()
        flex_h1_def().wait_send()

        for j, (u0, u1) in enumerate(k2_sends):
            with scope("recv_k2r_%d" % j):
                rdma("r", 2, j).wait_recv()
            accumulate(recv_l, 2, u0, u1, 0)
            with scope("recv_k2l_%d" % j):
                rdma("l", 2, j).wait_recv()
            accumulate(recv_r, 2, u0, u1, 1)
        with scope("sent_k2"):
            for j in range(len(k2_sends)):
                rdma("r", 2, j).wait_send()
                rdma("l", 2, j).wait_send()

    return pl.pallas_call(
        body,
        out_shape=jax.ShapeDtypeStruct((mb, n), f32),
        in_specs=[pl.BlockSpec(memory_space=pl.ANY), pl.BlockSpec(memory_space=pl.ANY)],
        out_specs=pl.BlockSpec(memory_space=pltpu.VMEM),
        scratch_shapes=[
            pltpu.VMEM((2, 2, qb, k), f32),
            pltpu.VMEM((6, 2, qb, k), f32),
            pltpu.VMEM((nt, k, T), f32),
            pltpu.VMEM((nt, k, T), bf16),
            pltpu.VMEM((3, nu, qb, T), bf16),
            pltpu.VMEM((3, nu, qb, T), bf16),
            pltpu.VMEM((3, nu, qb, T), bf16),
            pltpu.VMEM((3, nu, qb, T), bf16),
            pltpu.VMEM((NF, qb, T), bf16),
            pltpu.VMEM((NF, qb, T), bf16),
            pltpu.SemaphoreType.DMA((8,)),
            pltpu.SemaphoreType.DMA((nt,)),
            pltpu.SemaphoreType.DMA((n_rdma,)),
            pltpu.SemaphoreType.DMA((n_rdma,)),
            pltpu.SemaphoreType.DMA((n_rdma,)),
            pltpu.SemaphoreType.DMA((n_rdma,)),
            pltpu.SemaphoreType.DMA((2,)),
            pltpu.SemaphoreType.DMA((4,)),
        ],
        compiler_params=pltpu.CompilerParams(collective_id=0, disable_semaphore_checks=True,
                                             disable_bounds_checks=True,
                                             vmem_limit_bytes=64 * 1024 * 1024),
    )(A.reshape(N_DEV, 2, 2, qb, k), B)
```

```python
import jax
import jax.numpy as jnp
from jax import lax
from jax.experimental import pallas as pl
from jax.experimental.pallas import tpu as pltpu

N_DEV = 4
T = 128
E = 4
NF = 5


def pallas_dist_matmul_mk_i_outk_m1024_n1024_k512_kernel(
    A: jax.Array,
    B: jax.Array,
):
    m, k = A.shape
    _, n = B.shape
    mb = m // N_DEV
    hb = mb // 2
    ub = hb // E
    sb = ub // 2
    nt = n // T
    pt = 2 * E
    npc = pt * nt
    nfix = npc - 2 * NF
    bf16 = jnp.bfloat16
    f32 = jnp.float32

    k0_sends = [(2 * e, 2 * e + 2) for e in range(E)]
    k0_sends += [(pt, pt + 1), (pt + 1, pt + 2), (pt + 2, 2 * pt)]
    k0_sends += [(p, min(p + pt, nfix)) for p in range(2 * pt, nfix, pt)]
    k1_sends = [(0, 2 * pt), (2 * pt, 4 * pt), (4 * pt, nfix), (nfix, npc)]
    k2_sends = [(0, 4 * pt), (4 * pt, 6 * pt), (6 * pt, 7 * pt), (7 * pt, npc - 2), (npc - 2, npc)]
    sends = [k0_sends, k1_sends, k2_sends]
    sem_base = [0, len(k0_sends), len(k0_sends) + len(k1_sends)]
    n_rdma = sum(len(s) for s in sends)
    ends = [{p1: j for j, (_, p1) in enumerate(s)} for s in sends]

    def body(a_hbm, b_hbm, o_ref, ad_vm, a_vm, b_vm, b_bf, send_r, send_l, recv_l, recv_r,
             extra_l, extra_r, a_sems, b_sems, sr_sems, sl_sems, rl_sems, rr_sems, fs_sems, fr_sems):
        me = lax.axis_index("i")
        right = (me + 1) & (N_DEV - 1)
        left = (me + N_DEV - 1) & (N_DEV - 1)
        diag = me ^ 2

        def ad_copy(e):
            return pltpu.make_async_copy(a_hbm.at[diag, :, e], ad_vm.at[e], a_sems.at[e])

        a_src = [(right, 1), (left, 0), (right, 0), (left, 1), (me, 0), (me, 1)]

        def a_copy(s):
            blk, h = a_src[s]
            return pltpu.make_async_copy(a_hbm.at[blk, h], a_vm.at[s], a_sems.at[E + s])

        def b_copy(c):
            return pltpu.make_async_copy(b_hbm.at[:, pl.ds(c * T, T)], b_vm.at[c], b_sems.at[c])

        def remote(src, dst, ssem, rsem, dev):
            return pltpu.make_async_remote_copy(
                src_ref=src, dst_ref=dst, send_sem=ssem, recv_sem=rsem,
                device_id=(dev,), device_id_type=pl.DeviceIdType.MESH)

        def rdma(d, kind, j):
            p0, p1 = sends[kind][j]
            s = sem_base[kind] + j
            idx = (kind, pl.ds(p0, p1 - p0))
            if d == "r":
                return remote(send_r.at[idx], recv_l.at[idx], sr_sems.at[s], rl_sems.at[s], right)
            return remote(send_l.at[idx], recv_r.at[idx], sl_sems.at[s], rr_sems.at[s], left)

        fl = (0, pl.ds(nfix, 2 * NF))

        def flex(half, rerouted):
            if half == 0:
                if rerouted:
                    return remote(send_r.at[fl], extra_r, fs_sems.at[0], fr_sems.at[3], left)
                return remote(send_r.at[fl], recv_l.at[fl], fs_sems.at[0], fr_sems.at[0], right)
            if rerouted:
                return remote(send_l.at[fl], extra_l, fs_sems.at[1], fr_sems.at[2], right)
            return remote(send_l.at[fl], recv_r.at[fl], fs_sems.at[1], fr_sems.at[1], left)

        def put(d, kind, p, val):
            (send_r if d == "r" else send_l)[kind, p] = val
            if p + 1 in ends[kind]:
                rdma(d, kind, ends[kind][p + 1]).start()

        def b_cols(c0, c1):
            return jnp.concatenate([b_bf[c] for c in range(c0, c1)], axis=1)

        def lhs(s):
            return a_vm[pl.ds(s, 2)].reshape(mb, k).astype(bf16)

        def dot(x, y):
            return jnp.dot(x, y, preferred_element_type=f32)

        barrier = pltpu.get_barrier_semaphore()
        b_copy(0).start()
        for e in range(E):
            ad_copy(e).start()
        for nbr in (left, right):
            pl.semaphore_signal(barrier, inc=1, device_id=(nbr,), device_id_type=pl.DeviceIdType.MESH)
        for c in range(1, nt):
            b_copy(c).start()

        @pl.when(me == 0)
        def _():
            recv_l[0, pl.ds(nfix, 2 * NF)] = jnp.zeros((2 * NF, sb, T), bf16)
            recv_r[0, pl.ds(nfix, 2 * NF)] = jnp.zeros((2 * NF, sb, T), bf16)

        @pl.when(me != 2)
        def _():
            extra_l[...] = jnp.zeros((2 * NF, sb, T), bf16)
            extra_r[...] = jnp.zeros((2 * NF, sb, T), bf16)

        def put_strips(res, c, strips):
            for i, e in enumerate(strips):
                for d, off in (("r", 0), ("l", ub)):
                    for g in range(2):
                        r0 = i * 2 * ub + off + g * sb
                        put(d, 0, pt * c + 2 * e + g, res[r0:r0 + sb])

        b_copy(0).wait()
        for s in range(len(a_src)):
            a_copy(s).start()
        b_bf[0] = b_vm[0].astype(bf16)
        for e in range(E):
            ad_copy(e).wait()
            res = dot(ad_vm[e].reshape(2 * ub, k).astype(bf16), b_bf[0]).astype(bf16)
            if e == 0:
                pl.semaphore_wait(barrier, 2)
            put_strips(res, 0, [e])

        b_copy(1).wait()
        x = ad_vm[...].reshape(mb, k)
        x = jnp.concatenate([x[0:sb], x[ub:ub + sb], x[sb:ub], x[ub + sb:]], axis=0)
        res = dot(x.astype(bf16), b_vm[1].astype(bf16)).astype(bf16)
        for g in range(2):
            put("r", 0, pt + g, res[(2 * g) * sb:(2 * g + 1) * sb])
            put("l", 0, pt + g, res[(2 * g + 1) * sb:(2 * g + 2) * sb])
        put_strips(res[2 * ub:], 1, range(1, E))
        b_bf[1] = b_vm[1].astype(bf16)

        for c in range(2, nt):
            b_copy(c).wait()
            res = dot(ad_vm[...].reshape(mb, k).astype(bf16), b_vm[c].astype(bf16)).astype(bf16)
            put_strips(res, c, range(E))
            b_bf[c] = b_vm[c].astype(bf16)

        for half, rerouter in ((0, 3), (1, 1)):
            @pl.when(me != rerouter)
            def _():
                flex(half, False).start()

            @pl.when(me == rerouter)
            def _():
                flex(half, True).start()

        def pieces(res, c0, c1):
            for c in range(c0, c1):
                cc = slice((c - c0) * T, (c - c0 + 1) * T)
                for g in range(pt):
                    yield pt * c + g, res[g * sb:(g + 1) * sb, cc], res[hb + g * sb:hb + (g + 1) * sb, cc]

        a_copy(0).wait()
        a_copy(1).wait()
        for p0, p1 in k1_sends[:-1]:
            c0, c1 = p0 // pt, -(-p1 // pt)
            res = dot(lhs(0), b_cols(c0, c1))
            for p, vr, vl in pieces(res, c0, c1):
                if p < p1:
                    put("r", 1, p, vr.astype(bf16))
                    put("l", 1, p, vl.astype(bf16))

        a_copy(4).wait()
        a_copy(5).wait()
        o_ref[...] = dot(lhs(4), b_cols(0, nt))

        a_copy(2).wait()
        a_copy(3).wait()
        for j in range(len(k0_sends)):
            rdma("r", 0, j).wait_recv()
            rdma("l", 0, j).wait_recv()

        @pl.when(me != 0)
        def _():
            flex(0, False).wait_recv()
            flex(1, False).wait_recv()

        @pl.when(me == 2)
        def _():
            flex(0, True).wait_recv()
            flex(1, True).wait_recv()

        cf = nfix // pt
        res = dot(lhs(0), b_cols(cf, nt))
        for p, vr, vl in pieces(res, cf, nt):
            if p >= nfix:
                put("r", 1, p, (vr + extra_l[p - nfix].astype(f32)).astype(bf16))
                put("l", 1, p, (vl + extra_r[p - nfix].astype(f32)).astype(bf16))

        for c0, c1 in ((0, nt // 2), (nt // 2, nt)):
            res = dot(lhs(2), b_cols(c0, c1))
            for p, vr, vl in pieces(res, c0, c1):
                put("r", 2, p, (vr + recv_l[0, p].astype(f32)).astype(bf16))
                put("l", 2, p, (vl + recv_r[0, p].astype(f32)).astype(bf16))

        def accumulate(buf, kind, p0, p1, half):
            for p in range(p0, p1):
                rows = pl.ds(half * hb + (p % pt) * sb, sb)
                cols = pl.ds((p // pt) * T, T)
                o_ref[rows, cols] += buf[kind, p].astype(f32)

        for j, (p0, p1) in enumerate(k1_sends):
            rdma("r", 1, j).wait_recv()
            rdma("l", 1, j).wait_recv()
            accumulate(recv_r, 1, p0, p1, 0)
            accumulate(recv_l, 1, p0, p1, 1)

        for kind in range(2):
            for j in range(len(sends[kind])):
                rdma("r", kind, j).wait_send()
                rdma("l", kind, j).wait_send()
        flex(0, False).wait_send()
        flex(1, False).wait_send()

        for j, (p0, p1) in enumerate(k2_sends):
            order = (("r", recv_l, 0), ("l", recv_r, 1))
            if j == len(k2_sends) - 1:
                for i in range(len(k2_sends)):
                    rdma("r", 2, i).wait_send()
                    rdma("l", 2, i).wait_send()
                order = order[::-1]
            for d, buf, half in order:
                rdma(d, 2, j).wait_recv()
                accumulate(buf, 2, p0, p1, half)

    params = dict(collective_id=0, vmem_limit_bytes=32 * 1024 * 1024)
    if hasattr(pltpu.CompilerParams, "disable_semaphore_checks"):
        params["disable_semaphore_checks"] = True

    comm = pltpu.VMEM((3, npc, sb, T), bf16)
    return pl.pallas_call(
        body,
        out_shape=jax.ShapeDtypeStruct((mb, n), f32),
        in_specs=[pl.BlockSpec(memory_space=pl.ANY), pl.BlockSpec(memory_space=pl.ANY)],
        out_specs=pl.BlockSpec(memory_space=pltpu.VMEM),
        scratch_shapes=[
            pltpu.VMEM((E, 2, ub, k), f32),
            pltpu.VMEM((6, E, ub, k), f32),
            pltpu.VMEM((nt, k, T), f32),
            pltpu.VMEM((nt, k, T), bf16),
            comm, comm, comm, comm,
            pltpu.VMEM((2 * NF, sb, T), bf16),
            pltpu.VMEM((2 * NF, sb, T), bf16),
            pltpu.SemaphoreType.DMA((E + 6,)),
            pltpu.SemaphoreType.DMA((nt,)),
            pltpu.SemaphoreType.DMA((n_rdma,)),
            pltpu.SemaphoreType.DMA((n_rdma,)),
            pltpu.SemaphoreType.DMA((n_rdma,)),
            pltpu.SemaphoreType.DMA((n_rdma,)),
            pltpu.SemaphoreType.DMA((2,)),
            pltpu.SemaphoreType.DMA((4,)),
        ],
        compiler_params=pltpu.CompilerParams(**params),
    )(A.reshape(N_DEV, 2, E, ub, k), B)
```
